```python
import numpy as np

kernel_name = "dist_sum_ax0_xy_m2048_n1024"

def setup_inputs():
    return {"x": np.random.randn(4096, 2048).astype(np.float32)}

def reference(x: np.ndarray) -> np.ndarray:
    return np.sum(x, axis=0, keepdims=True)
```

```python
import jax
import jax.numpy as jnp
from jax import lax
from jax.experimental import pallas as pl
from jax.experimental.pallas import tpu as pltpu

_MESH = pl.DeviceIdType.MESH

_RAW_ROWS = 112
_FIRST_CHUNK = 1536
_WIDE_ROWS = (96, 32)
_NARROW = 128
_UNROLL = 64


def _accumulate(ref, row0, nrows, acc, unroll):
    width = acc.shape[1]

    def add(a, start, rows):
        blk = ref[pl.ds(start, rows), :]
        return a + jnp.sum(blk.reshape(rows // 8, 8, width), axis=0)

    if nrows <= unroll:
        return add(acc, row0, nrows)
    full = nrows // unroll
    acc = lax.fori_loop(
        0, full, lambda j, a: add(a, pl.multiple_of(row0 + j * unroll, 8), unroll), acc
    )
    if nrows % unroll:
        acc = add(acc, row0 + full * unroll, nrows % unroll)
    return acc


def pallas_dist_sum_ax0_xy_m2048_n1024_kernel(x: jax.Array):
    m, n = x.shape
    tail = sum(_WIDE_ROWS)
    main = m - _RAW_ROWS - tail
    chunks = ((0, _FIRST_CHUNK), (_FIRST_CHUNK, main - _FIRST_CHUNK))
    wide = n - _NARROW

    def body(x_hbm, out_ref, buf, wide_buf, narrow_buf, raw_buf, send_buf, recv_buf,
             sems, send_sems, recv_sems):
        main_copies = [
            pltpu.make_async_copy(x_hbm.at[pl.ds(o, s)], buf.at[pl.ds(o, s)], sems.at[i])
            for i, (o, s) in enumerate(chunks)
        ]
        wide_copies = []
        o = 0
        for i, s in enumerate(_WIDE_ROWS):
            wide_copies.append((o, s, pltpu.make_async_copy(
                x_hbm.at[pl.ds(main + o, s), pl.ds(0, wide)], wide_buf.at[pl.ds(o, s)],
                sems.at[len(chunks) + i])))
            o += s
        k = len(chunks) + len(_WIDE_ROWS)
        narrow_copy = pltpu.make_async_copy(
            x_hbm.at[pl.ds(main, tail), pl.ds(wide, _NARROW)], narrow_buf, sems.at[k])
        for c in main_copies:
            c.start()
        for _, _, c in wide_copies:
            c.start()
        narrow_copy.start()

        my_x = lax.axis_index("x")
        peer = (1 - my_x, lax.axis_index("y"))
        barrier = pltpu.get_barrier_semaphore()
        pl.semaphore_signal(barrier, inc=1, device_id=peer, device_id_type=_MESH)

        last_rows = x_hbm.at[pl.ds(m - _RAW_ROWS, _RAW_ROWS)]
        own_copy = pltpu.make_async_copy(
            last_rows, raw_buf.at[pl.ds(0, _RAW_ROWS)], sems.at[k + 1])
        raw_copy = pltpu.make_async_remote_copy(
            last_rows, raw_buf.at[pl.ds(_RAW_ROWS, _RAW_ROWS)],
            send_sems.at[2], recv_sems.at[2], device_id=peer, device_id_type=_MESH)

        @pl.when(my_x == 0)
        def _():
            own_copy.start()

        pl.semaphore_wait(barrier, 1)

        @pl.when(my_x == 1)
        def _():
            raw_copy.start()

        acc = jnp.zeros((8, n), jnp.float32)
        for (o, s), c in zip(chunks, main_copies):
            c.wait()
            acc = _accumulate(buf, o, s, acc, _UNROLL)

        def receiver(a):
            own_copy.wait()
            raw_copy.wait_recv()
            return _accumulate(raw_buf, 0, 2 * _RAW_ROWS, a, _UNROLL)

        def sender(a):
            raw_copy.wait_send()
            return a

        acc = lax.cond(my_x == 0, receiver, sender, acc)

        def swap(col, cols, i):
            return pltpu.make_async_remote_copy(
                send_buf.at[:, pl.ds(col, cols)], recv_buf.at[:, pl.ds(col, cols)],
                send_sems.at[i], recv_sems.at[i], device_id=peer, device_id_type=_MESH)

        swap_wide, swap_narrow = swap(0, wide, 0), swap(wide, _NARROW, 1)
        acc_wide, acc_narrow = acc[:, :wide], acc[:, wide:]
        for o, s, c in wide_copies:
            c.wait()
            acc_wide = _accumulate(wide_buf, o, s, acc_wide, tail)
        sum_wide = jnp.sum(acc_wide, axis=0, keepdims=True)
        send_buf[:, pl.ds(0, wide)] = sum_wide
        swap_wide.start()
        narrow_copy.wait()
        acc_narrow = _accumulate(narrow_buf, 0, tail, acc_narrow, tail)
        sum_narrow = jnp.sum(acc_narrow, axis=0, keepdims=True)
        send_buf[:, pl.ds(wide, _NARROW)] = sum_narrow
        swap_narrow.start()

        swap_wide.wait_send()
        swap_narrow.wait_send()
        swap_wide.wait_recv()
        out_ref[:, pl.ds(0, wide)] = sum_wide + recv_buf[:, pl.ds(0, wide)]
        swap_narrow.wait_recv()
        out_ref[:, pl.ds(wide, _NARROW)] = sum_narrow + recv_buf[:, pl.ds(wide, _NARROW)]

    return pl.pallas_call(
        body,
        out_shape=jax.ShapeDtypeStruct((1, n), jnp.float32),
        in_specs=[pl.BlockSpec(memory_space=pl.ANY)],
        out_specs=pl.BlockSpec(memory_space=pltpu.VMEM),
        scratch_shapes=[
            pltpu.VMEM((main, n), jnp.float32),
            pltpu.VMEM((tail, wide), jnp.float32),
            pltpu.VMEM((tail, _NARROW), jnp.float32),
            pltpu.VMEM((2 * _RAW_ROWS, n), jnp.float32),
            pltpu.VMEM((1, n), jnp.float32),
            pltpu.VMEM((1, n), jnp.float32),
            pltpu.SemaphoreType.DMA((len(chunks) + len(_WIDE_ROWS) + 2,)),
            pltpu.SemaphoreType.DMA((3,)),
            pltpu.SemaphoreType.DMA((3,)),
        ],
        compiler_params=pltpu.CompilerParams(
            collective_id=0,
            disable_semaphore_checks=True,
            disable_bounds_checks=True,
        ),
    )(x)
```

```python
import jax
import jax.numpy as jnp
from jax import lax
from jax.experimental import pallas as pl
from jax.experimental.pallas import tpu as pltpu

X_ROWS = 120
Y_ROWS = 80
TAIL_ROWS = 192
NARROW = 128
FIRST_ROWS = 1024
LAST_ROWS = 24
LOOP_ROWS = 64

_SUBLANES = 8
_MESH = pl.DeviceIdType.MESH


def _add_rows(acc, ref, start, rows):
    def add(total, first, count):
        block = ref[pl.ds(first, count), :]
        return total + jnp.sum(block.reshape(-1, _SUBLANES, block.shape[1]), axis=0)

    def step(i, total):
        first = pl.multiple_of(start + i * LOOP_ROWS, _SUBLANES)
        return add(total, first, LOOP_ROWS)

    steps, rest = divmod(rows, LOOP_ROWS)
    if steps:
        acc = lax.fori_loop(0, steps, step, acc)
    if rest:
        acc = add(acc, start + steps * LOOP_ROWS, rest)
    return acc


def _add_rows_tree(acc, ref, start, rows):
    terms = [ref[pl.ds(start + r, _SUBLANES), :] for r in range(0, rows, _SUBLANES)]
    terms.append(acc)
    while len(terms) > 1:
        pairs = [a + b for a, b in zip(terms[0::2], terms[1::2])]
        terms = pairs + terms[2 * len(pairs) :]
    return terms[0]


def pallas_dist_sum_ax0_xy_m2048_n1024_kernel(x: jax.Array):
    m, n = x.shape
    wide = n - NARROW
    main_rows = m - TAIL_ROWS - Y_ROWS - X_ROWS
    tail_start = 0
    main_start = tail_start + TAIL_ROWS
    y_start = main_start + main_rows
    x_start = y_start + Y_ROWS

    def body(
        x_hbm, out_ref,
        main_buf, wide_buf, narrow_buf, kept_buf, streamed_buf,
        y_sum_out, y_sum_in, wide_out, wide_in, narrow_out, narrow_in,
        read_sems, send_sems, recv_sems, helper_ready,
    ):
        def read(src_start, cols, buf, start, rows, sem):
            return pltpu.make_async_copy(
                x_hbm.at[pl.ds(src_start + start, rows), cols],
                buf.at[pl.ds(start, rows)],
                read_sems.at[sem],
            )

        early_rows = TAIL_ROWS - LAST_ROWS
        all_cols, wide_cols, narrow_cols = pl.ds(0, n), pl.ds(0, wide), pl.ds(wide, NARROW)
        main_0 = read(main_start, all_cols, main_buf, 0, FIRST_ROWS, 0)
        main_1 = read(main_start, all_cols, main_buf, FIRST_ROWS, main_rows - FIRST_ROWS, 1)
        wide_0 = read(tail_start, wide_cols, wide_buf, 0, early_rows, 2)
        wide_1 = read(tail_start, wide_cols, wide_buf, early_rows, LAST_ROWS, 3)
        narrow_0 = read(tail_start, narrow_cols, narrow_buf, 0, early_rows, 4)
        narrow_1 = read(tail_start, narrow_cols, narrow_buf, early_rows, LAST_ROWS, 5)
        for copy in (main_0, main_1, wide_0, wide_1, narrow_0, narrow_1):
            copy.start()

        my_x, my_y = lax.axis_index("x"), lax.axis_index("y")
        peer, side = (1 - my_x, my_y), (my_x, 1 - my_y)
        is_x0 = my_x == 0
        is_lead = jnp.logical_and(my_x == 1, my_y == 0)
        is_helper = jnp.logical_and(my_x == 1, my_y == 1)

        def remote(src, dst, target, sem):
            return pltpu.make_async_remote_copy(
                src, dst, send_sems.at[sem], recv_sems.at[sem],
                device_id=target, device_id_type=_MESH,
            )

        wide_swap = remote(wide_out, wide_in, peer, 0)
        narrow_swap = remote(narrow_out, narrow_in, peer, 1)
        x_stream = remote(x_hbm.at[pl.ds(x_start, X_ROWS)], streamed_buf, peer, 2)
        y_stream = remote(
            x_hbm.at[pl.ds(y_start, Y_ROWS)], streamed_buf.at[pl.ds(0, Y_ROWS)], side, 3
        )
        y_sum = remote(y_sum_out, y_sum_in, side, 4)
        kept_yx = read(y_start, all_cols, kept_buf, 0, Y_ROWS + X_ROWS, 6)
        kept_y = read(y_start, all_cols, kept_buf, 0, Y_ROWS, 6)
        zeros = jnp.zeros((_SUBLANES, n), jnp.float32)

        barrier = pltpu.get_barrier_semaphore()
        pl.semaphore_signal(barrier, 1, device_id=peer, device_id_type=_MESH)

        @pl.when(is_x0)
        def _():
            kept_yx.start()
            pl.semaphore_wait(barrier, 1)

        @pl.when(is_lead)
        def _():
            pl.semaphore_signal(barrier, 1, device_id=side, device_id_type=_MESH)
            pl.semaphore_wait(barrier, 1)
            x_stream.start()
            pl.semaphore_wait(helper_ready, 1)
            y_stream.start()

        @pl.when(is_helper)
        def _():
            kept_y.start()
            pl.semaphore_wait(barrier, 2)
            pl.semaphore_signal(helper_ready, 1, device_id=side, device_id_type=_MESH)
            x_stream.start()
            y_stream.wait_recv()
            total = _add_rows(zeros, streamed_buf, 0, Y_ROWS)
            y_sum_out[...] = jnp.sum(total, axis=0, keepdims=True)
            y_sum.start()

        main_0.wait()
        acc = _add_rows(zeros, main_buf, 0, FIRST_ROWS)
        main_1.wait()
        acc = _add_rows(acc, main_buf, FIRST_ROWS, main_rows - FIRST_ROWS)
        wide_0.wait()
        acc_wide = _add_rows(acc[:, :wide], wide_buf, 0, early_rows)

        def rest_of_x0():
            kept_yx.wait()
            total = _add_rows(zeros, kept_buf, 0, Y_ROWS + X_ROWS)
            x_stream.wait_recv()
            return _add_rows(total, streamed_buf, 0, X_ROWS)

        def rest_of_lead():
            y_sum.wait_recv()
            top_row = lax.broadcasted_iota(jnp.int32, zeros.shape, 0) == 0
            return jnp.where(top_row, y_sum_in[...], zeros)

        def rest_of_helper():
            kept_y.wait()
            return _add_rows(zeros, kept_buf, 0, Y_ROWS)

        rest = lax.cond(
            is_x0, rest_of_x0, lambda: lax.cond(is_lead, rest_of_lead, rest_of_helper)
        )
        acc_wide = acc_wide + rest[:, :wide]
        acc_narrow = acc[:, wide:] + rest[:, wide:]

        wide_1.wait()
        acc_wide = _add_rows_tree(acc_wide, wide_buf, early_rows, LAST_ROWS)
        wide_out[...] = jnp.sum(acc_wide, axis=0, keepdims=True)
        wide_swap.start()

        narrow_0.wait()
        acc_narrow = _add_rows_tree(acc_narrow, narrow_buf, 0, early_rows)
        narrow_1.wait()
        acc_narrow = _add_rows_tree(acc_narrow, narrow_buf, early_rows, LAST_ROWS)
        narrow_out[...] = jnp.sum(acc_narrow, axis=0, keepdims=True)
        narrow_swap.start()

        wide_swap.wait_send()
        narrow_swap.wait_send()

        @pl.when(is_lead)
        def _():
            x_stream.wait_send()
            y_stream.wait_send()

        @pl.when(is_helper)
        def _():
            x_stream.wait_send()
            y_sum.wait_send()

        wide_swap.wait_recv()
        out_ref[:, wide_cols] = wide_out[...] + wide_in[...]
        narrow_swap.wait_recv()
        out_ref[:, narrow_cols] = narrow_out[...] + narrow_in[...]

    def vmem(rows, cols):
        return pltpu.VMEM((rows, cols), jnp.float32)

    return pl.pallas_call(
        body,
        out_shape=jax.ShapeDtypeStruct((1, n), jnp.float32),
        in_specs=[pl.BlockSpec(memory_space=pl.ANY)],
        out_specs=pl.BlockSpec(memory_space=pltpu.VMEM),
        scratch_shapes=[
            vmem(main_rows, n),
            vmem(TAIL_ROWS, wide),
            vmem(TAIL_ROWS, NARROW),
            vmem(Y_ROWS + X_ROWS, n),
            vmem(X_ROWS, n),
            vmem(1, n),
            vmem(1, n),
            vmem(1, wide),
            vmem(1, wide),
            vmem(1, NARROW),
            vmem(1, NARROW),
            pltpu.SemaphoreType.DMA((7,)),
            pltpu.SemaphoreType.DMA((5,)),
            pltpu.SemaphoreType.DMA((5,)),
            pltpu.SemaphoreType.REGULAR,
        ],
        compiler_params=pltpu.CompilerParams(
            collective_id=0, disable_semaphore_checks=True
        ),
    )(x)
```

```python
import jax
import jax.numpy as jnp
from jax import lax
from jax.experimental import pallas as pl
from jax.experimental.pallas import tpu as pltpu

SUBLANES, LANES = 8, 128
HEAD = 7
UNIT = 16
SWEEPS = 8
LEFT_UNITS = 11
Y_TILES = 72
LAST_UNITS = 2

_MESH = pl.DeviceIdType.MESH


def _sum_groups(tiles, group):
    return jnp.sum(tiles.reshape(-1, group, SUBLANES, LANES), axis=0)


def _tree_sum(terms):
    while len(terms) > 1:
        pairs = [a + b for a, b in zip(terms[0::2], terms[1::2])]
        terms = pairs + terms[2 * len(pairs) :]
    return terms[0]


def _to_row(tiles):
    rows = [jnp.sum(tiles[i], axis=0, keepdims=True) for i in range(tiles.shape[0])]
    return jnp.concatenate(rows, axis=1)


def pallas_dist_sum_ax0_xy_m2048_n1024_kernel(x: jax.Array):
    m, n = x.shape
    cols = n // LANES
    tiles = m // SUBLANES * cols
    assert HEAD == cols - 1 and UNIT % cols == 0 and Y_TILES % cols == 0
    x_tiles = (
        x.reshape(m // SUBLANES, SUBLANES, cols, LANES)
        .transpose(0, 2, 1, 3)
        .reshape(tiles, SUBLANES, LANES)
    )
    wide = n - LANES
    runs = UNIT // cols
    period = SWEEPS * UNIT
    swept_units = (tiles - HEAD) // UNIT - LEFT_UNITS
    units = [len(range(j, swept_units, SWEEPS)) for j in range(SWEEPS)]
    early_units = units[0] - LAST_UNITS
    y_start = HEAD + swept_units * UNIT
    x_start = y_start + Y_TILES
    x_count = tiles - x_start

    def body(
        x_hbm, out_ref,
        swept_buf, wide_buf, narrow_buf, kept_buf, streamed_buf, head_buf,
        y_sum_out, y_sum_in, wide_out, wide_in, narrow_out, narrow_in,
        sweep_sems, read_sems, send_sems, recv_sems, helper_ready,
    ):
        def sweep(j):
            src = x_hbm.at[pl.ds(HEAD, units[j] * period)]
            src = src.reshape(units[j], period, SUBLANES, LANES)
            return pltpu.make_async_copy(
                src.at[:, pl.ds(j * UNIT, UNIT)],
                swept_buf.at[j - 1, pl.ds(0, units[j])],
                sweep_sems.at[j - 1],
            )

        def slab(buf, col, width, first, count, sem):
            src = x_hbm.at[pl.ds(HEAD + first * period, count * period)]
            src = src.reshape(count, period // cols, cols, SUBLANES, LANES)
            return pltpu.make_async_copy(
                src.at[:, pl.ds(0, runs), pl.ds(col, width)],
                buf.at[pl.ds(first, count)],
                read_sems.at[sem],
            )

        sweeps = [sweep(j) for j in range(1, SWEEPS)]
        wide_0 = slab(wide_buf, 1, cols - 1, 0, early_units, 0)
        wide_1 = slab(wide_buf, 1, cols - 1, early_units, LAST_UNITS, 1)
        narrow_0 = slab(narrow_buf, 0, 1, 0, early_units, 2)
        narrow_1 = slab(narrow_buf, 0, 1, early_units, LAST_UNITS, 3)
        for copy in (*sweeps, wide_0, wide_1, narrow_0, narrow_1):
            copy.start()

        my_x, my_y = lax.axis_index("x"), lax.axis_index("y")
        peer, side = (1 - my_x, my_y), (my_x, 1 - my_y)
        is_x0 = my_x == 0
        is_lead = jnp.logical_and(my_x == 1, my_y == 0)
        is_helper = jnp.logical_and(my_x == 1, my_y == 1)

        def local(start, count, dst, sem):
            src = x_hbm.at[pl.ds(start, count)]
            return pltpu.make_async_copy(src, dst, read_sems.at[sem])

        def remote(src, dst, target, sem):
            return pltpu.make_async_remote_copy(
                src, dst, send_sems.at[sem], recv_sems.at[sem],
                device_id=target, device_id_type=_MESH,
            )

        wide_swap = remote(wide_out, wide_in, peer, 0)
        narrow_swap = remote(narrow_out, narrow_in, peer, 1)
        x_stream = remote(x_hbm.at[pl.ds(x_start, x_count)], streamed_buf, peer, 2)
        head_stream = remote(x_hbm.at[pl.ds(0, HEAD)], head_buf, peer, 3)
        y_stream = remote(
            x_hbm.at[pl.ds(y_start, Y_TILES)], streamed_buf.at[pl.ds(0, Y_TILES)], side, 4
        )
        y_sum = remote(y_sum_out, y_sum_in, side, 5)
        kept_yx = local(y_start, Y_TILES + x_count, kept_buf.at[pl.ds(0, Y_TILES + x_count)], 4)
        kept_head = local(0, HEAD, kept_buf.at[pl.ds(Y_TILES + x_count, HEAD)], 5)
        kept_y = local(y_start, Y_TILES, kept_buf.at[pl.ds(0, Y_TILES)], 6)
        own_head = local(0, HEAD, head_buf, 7)

        barrier = pltpu.get_barrier_semaphore()
        pl.semaphore_signal(barrier, 1, device_id=peer, device_id_type=_MESH)

        @pl.when(is_x0)
        def _():
            kept_yx.start()
            kept_head.start()
            pl.semaphore_wait(barrier, 1)

        @pl.when(is_lead)
        def _():
            pl.semaphore_signal(barrier, 1, device_id=side, device_id_type=_MESH)
            pl.semaphore_wait(barrier, 1)
            x_stream.start()
            head_stream.start()
            pl.semaphore_wait(helper_ready, 1)
            y_stream.start()

        @pl.when(is_helper)
        def _():
            kept_y.start()
            pl.semaphore_wait(barrier, 2)
            pl.semaphore_signal(helper_ready, 1, device_id=side, device_id_type=_MESH)
            x_stream.start()
            head_stream.start()
            y_stream.wait_recv()
            y_sum_out[...] = _to_row(_sum_groups(streamed_buf[pl.ds(0, Y_TILES)], cols))
            y_sum.start()

        acc = jnp.zeros((cols, SUBLANES, LANES), jnp.float32)
        for j, copy in enumerate(sweeps, start=1):
            copy.wait()
            acc = acc + _sum_groups(swept_buf[j - 1, pl.ds(0, units[j])], cols)
        wide_0.wait()
        acc_wide = acc[1:] + _sum_groups(wide_buf[pl.ds(0, early_units)], cols - 1)

        def rest_of_x0():
            kept_yx.wait()
            kept_head.wait()
            total = _sum_groups(kept_buf[...], cols)
            x_stream.wait_recv()
            total = total + _sum_groups(streamed_buf[pl.ds(0, x_count - 1)], cols)
            return total[1:], total[0] + streamed_buf[x_count - 1]

        def rest_of_lead():
            y_sum.wait_recv()
            top = lax.broadcasted_iota(jnp.int32, (SUBLANES, LANES), 0) == 0
            total = [
                jnp.where(top, y_sum_in[:, pl.ds(i * LANES, LANES)], 0.0)
                for i in range(cols)
            ]
            return jnp.stack(total[1:]), total[0]

        def rest_of_helper():
            kept_y.wait()
            total = _sum_groups(kept_buf[pl.ds(0, Y_TILES)], cols)
            return total[1:], total[0]

        rest_wide, rest_narrow = lax.cond(
            is_x0, rest_of_x0, lambda: lax.cond(is_lead, rest_of_lead, rest_of_helper)
        )
        acc_wide = acc_wide + rest_wide
        acc_narrow = acc[0] + rest_narrow

        early = [(u, r) for u in range(early_units) for r in range(runs)]
        last = [(u, r) for u in range(early_units, units[0]) for r in range(runs)]
        wide_1.wait()
        wide_out[...] = _to_row(_tree_sum([wide_buf[u, r] for u, r in last] + [acc_wide]))
        wide_swap.start()
        narrow_0.wait()
        acc_narrow = _tree_sum([narrow_buf[u, r, 0] for u, r in early] + [acc_narrow])
        narrow_1.wait()
        acc_narrow = _tree_sum([narrow_buf[u, r, 0] for u, r in last] + [acc_narrow])
        narrow_out[...] = jnp.sum(acc_narrow, axis=0, keepdims=True)
        narrow_swap.start()

        @pl.when(my_x == 1)
        def _():
            own_head.start()
            own_head.wait()
            x_stream.wait_send()
            head_stream.wait_send()

        @pl.when(is_lead)
        def _():
            y_stream.wait_send()

        @pl.when(is_helper)
        def _():
            y_sum.wait_send()

        wide_swap.wait_send()
        narrow_swap.wait_send()

        @pl.when(is_x0)
        def _():
            head_stream.wait_recv()

        own_wide = wide_out[...] + _to_row(head_buf[...])
        wide_swap.wait_recv()
        out_ref[:, pl.ds(0, wide)] = own_wide + wide_in[...]
        narrow_swap.wait_recv()
        out_ref[:, pl.ds(wide, LANES)] = narrow_out[...] + narrow_in[...]

    def vmem(*shape):
        return pltpu.VMEM(shape, jnp.float32)

    return pl.pallas_call(
        body,
        out_shape=jax.ShapeDtypeStruct((1, n), jnp.float32),
        in_specs=[pl.BlockSpec(memory_space=pl.ANY)],
        out_specs=pl.BlockSpec(memory_space=pltpu.VMEM),
        scratch_shapes=[
            vmem(SWEEPS - 1, max(units), UNIT, SUBLANES, LANES),
            vmem(units[0], runs, cols - 1, SUBLANES, LANES),
            vmem(units[0], runs, 1, SUBLANES, LANES),
            vmem(Y_TILES + x_count + HEAD, SUBLANES, LANES),
            vmem(x_count, SUBLANES, LANES),
            vmem(HEAD, SUBLANES, LANES),
            vmem(1, n),
            vmem(1, n),
            vmem(1, wide),
            vmem(1, wide),
            vmem(1, LANES),
            vmem(1, LANES),
            pltpu.SemaphoreType.DMA((SWEEPS - 1,)),
            pltpu.SemaphoreType.DMA((8,)),
            pltpu.SemaphoreType.DMA((6,)),
            pltpu.SemaphoreType.DMA((6,)),
            pltpu.SemaphoreType.REGULAR,
        ],
        compiler_params=pltpu.CompilerParams(
            collective_id=0, disable_semaphore_checks=True
        ),
    )(x_tiles)
```

```python
import jax
import jax.numpy as jnp
from jax import lax
from jax.experimental import pallas as pl
from jax.experimental.pallas import tpu as pltpu

SUBLANES, LANES = 8, 128
HEAD = 7
UNIT = 16
SWEEPS = 8
LEFT_UNITS = 11
Y_TILES = 72
LAST_UNITS = 2

_MESH = pl.DeviceIdType.MESH


def _sum_groups(tiles, group):
    return jnp.sum(tiles.reshape(-1, group, SUBLANES, LANES), axis=0)


def _tree_sum(terms):
    while len(terms) > 1:
        pairs = [a + b for a, b in zip(terms[0::2], terms[1::2])]
        terms = pairs + terms[2 * len(pairs) :]
    return terms[0]


def _to_row(tiles):
    rows = [jnp.sum(tiles[i], axis=0, keepdims=True) for i in range(tiles.shape[0])]
    return jnp.concatenate(rows, axis=1)


def pallas_dist_sum_ax0_xy_m2048_n1024_kernel(x: jax.Array):
    m, n = x.shape
    cols = n // LANES
    tiles = m // SUBLANES * cols
    wide = n - LANES
    runs = UNIT // cols
    period = SWEEPS * UNIT
    assert HEAD == cols - 1 and UNIT % cols == 0 and Y_TILES % cols == 0
    x_tiles = (
        x.reshape(m // SUBLANES, SUBLANES, cols, LANES)
        .transpose(0, 2, 1, 3)
        .reshape(tiles, SUBLANES, LANES)
    )
    x_periods = x_tiles.reshape(tiles // period, period, SUBLANES, LANES)
    x_rows = x_tiles.reshape(tiles // period, period // cols, cols, SUBLANES, LANES)
    swept_units = (tiles - HEAD) // UNIT - LEFT_UNITS
    units = [len(range(j, swept_units, SWEEPS)) for j in range(SWEEPS)]
    early_units = units[0] - LAST_UNITS
    y_start = HEAD + swept_units * UNIT
    x_start = y_start + Y_TILES
    x_count = tiles - x_start

    def body(
        tiles_hbm, periods_hbm, rows_hbm, out_ref,
        swept_buf, wide_buf, narrow_buf, kept_buf, streamed_buf, head_buf,
        y_sum_out, y_sum_in, wide_out, wide_in, narrow_out, narrow_in,
        sweep_sems, read_sems, send_sems, recv_sems, helper_ready,
    ):
        def local(start, count, dst, sem):
            return pltpu.make_async_copy(tiles_hbm.at[pl.ds(start, count)], dst, sem)

        def sweep(j):
            start, count, sem = HEAD + j * UNIT, units[j], sweep_sems.at[j - 1]
            if start + UNIT <= period:
                src = periods_hbm.at[pl.ds(0, count), pl.ds(start, UNIT)]
                dst = swept_buf.at[j - 1, pl.ds(0, count)]
                return [pltpu.make_async_copy(src, dst, sem)]
            return [
                local(start + u * period, UNIT, swept_buf.at[j - 1, u], sem)
                for u in range(count)
            ]

        def slab(buf, row, col, width, first, count, sem):
            src = rows_hbm.at[pl.ds(first, count), pl.ds(row, runs), pl.ds(col, width)]
            return pltpu.make_async_copy(src, buf.at[pl.ds(first, count)], read_sems.at[sem])

        sweeps = [sweep(j) for j in range(1, SWEEPS)]
        wide_0 = slab(wide_buf, 1, 0, cols - 1, 0, early_units, 0)
        wide_1 = slab(wide_buf, 1, 0, cols - 1, early_units, LAST_UNITS, 1)
        narrow_0 = slab(narrow_buf, 0, cols - 1, 1, 0, early_units, 2)
        narrow_1 = slab(narrow_buf, 0, cols - 1, 1, early_units, LAST_UNITS, 3)
        for copies in sweeps[:-1]:
            for copy in copies:
                copy.start()

        def start_last_reads():
            for copy in (*sweeps[-1], wide_0, wide_1, narrow_0, narrow_1):
                copy.start()

        my_x, my_y = lax.axis_index("x"), lax.axis_index("y")
        peer, side = (1 - my_x, my_y), (my_x, 1 - my_y)
        is_x0 = my_x == 0
        is_lead = jnp.logical_and(my_x == 1, my_y == 0)
        is_helper = jnp.logical_and(my_x == 1, my_y == 1)

        def remote(src, dst, target, sem):
            return pltpu.make_async_remote_copy(
                src, dst, send_sems.at[sem], recv_sems.at[sem],
                device_id=target, device_id_type=_MESH,
            )

        wide_swap = remote(wide_out, wide_in, peer, 0)
        narrow_swap = remote(narrow_out, narrow_in, peer, 1)
        x_stream = remote(tiles_hbm.at[pl.ds(x_start, x_count)], streamed_buf, peer, 2)
        head_stream = remote(tiles_hbm.at[pl.ds(0, HEAD)], head_buf, peer, 3)
        y_stream = remote(
            tiles_hbm.at[pl.ds(y_start, Y_TILES)], streamed_buf.at[pl.ds(0, Y_TILES)], side, 4
        )
        y_sum = remote(y_sum_out, y_sum_in, side, 5)
        kept_yx = local(y_start, Y_TILES + x_count, kept_buf.at[pl.ds(0, Y_TILES + x_count)], read_sems.at[4])
        kept_head = local(0, HEAD, kept_buf.at[pl.ds(Y_TILES + x_count, HEAD)], read_sems.at[5])
        kept_y = local(y_start, Y_TILES, kept_buf.at[pl.ds(0, Y_TILES)], read_sems.at[6])
        own_head = local(0, HEAD, head_buf, read_sems.at[7])

        barrier = pltpu.get_barrier_semaphore()
        pl.semaphore_signal(barrier, 1, device_id=peer, device_id_type=_MESH)

        @pl.when(is_x0)
        def _():
            start_last_reads()
            kept_yx.start()
            kept_head.start()
            pl.semaphore_wait(barrier, 1)

        @pl.when(is_lead)
        def _():
            pl.semaphore_signal(barrier, 1, device_id=side, device_id_type=_MESH)
            pl.semaphore_wait(barrier, 1)
            x_stream.start()
            head_stream.start()
            pl.semaphore_wait(helper_ready, 1)
            y_stream.start()
            start_last_reads()

        @pl.when(is_helper)
        def _():
            pl.semaphore_wait(barrier, 2)
            pl.semaphore_signal(helper_ready, 1, device_id=side, device_id_type=_MESH)
            x_stream.start()
            head_stream.start()
            start_last_reads()
            kept_y.start()
            y_stream.wait_recv()
            y_sum_out[...] = _to_row(_sum_groups(streamed_buf[pl.ds(0, Y_TILES)], cols))
            y_sum.start()

        acc = jnp.zeros((cols, SUBLANES, LANES), jnp.float32)
        for j, copies in enumerate(sweeps, start=1):
            for copy in copies:
                copy.wait()
            acc = acc + _sum_groups(swept_buf[j - 1, pl.ds(0, units[j])], cols)
        wide_0.wait()
        acc_wide = acc[1:] + _sum_groups(wide_buf[pl.ds(0, early_units)], cols - 1)

        def rest_of_x0():
            kept_yx.wait()
            kept_head.wait()
            total = _sum_groups(kept_buf[...], cols)
            x_stream.wait_recv()
            total = total + _sum_groups(streamed_buf[pl.ds(0, x_count - 1)], cols)
            return total[1:], total[0] + streamed_buf[x_count - 1]

        def rest_of_lead():
            y_sum.wait_recv()
            top = lax.broadcasted_iota(jnp.int32, (SUBLANES, LANES), 0) == 0
            total = [
                jnp.where(top, y_sum_in[:, pl.ds(i * LANES, LANES)], 0.0)
                for i in range(cols)
            ]
            return jnp.stack(total[1:]), total[0]

        def rest_of_helper():
            kept_y.wait()
            total = _sum_groups(kept_buf[pl.ds(0, Y_TILES)], cols)
            return total[1:], total[0]

        rest_wide, rest_narrow = lax.cond(
            is_x0, rest_of_x0, lambda: lax.cond(is_lead, rest_of_lead, rest_of_helper)
        )
        acc_wide = acc_wide + rest_wide
        acc_narrow = acc[0] + rest_narrow

        early = [(u, r) for u in range(early_units) for r in range(runs)]
        last = [(u, r) for u in range(early_units, units[0]) for r in range(runs)]
        wide_1.wait()
        wide_out[...] = _to_row(_tree_sum([wide_buf[u, r] for u, r in last] + [acc_wide]))
        wide_swap.start()
        narrow_0.wait()
        acc_narrow = _tree_sum([narrow_buf[u, r, 0] for u, r in early] + [acc_narrow])
        narrow_1.wait()
        acc_narrow = _tree_sum([narrow_buf[u, r, 0] for u, r in last] + [acc_narrow])
        narrow_out[...] = jnp.sum(acc_narrow, axis=0, keepdims=True)
        narrow_swap.start()

        @pl.when(my_x == 1)
        def _():
            own_head.start()
            own_head.wait()
            x_stream.wait_send()
            head_stream.wait_send()

        @pl.when(is_lead)
        def _():
            y_stream.wait_send()

        @pl.when(is_helper)
        def _():
            y_sum.wait_send()

        wide_swap.wait_send()
        narrow_swap.wait_send()

        @pl.when(is_x0)
        def _():
            head_stream.wait_recv()

        own_wide = wide_out[...] + _to_row(head_buf[...])
        wide_swap.wait_recv()
        out_ref[:, pl.ds(0, wide)] = own_wide + wide_in[...]
        narrow_swap.wait_recv()
        out_ref[:, pl.ds(wide, LANES)] = narrow_out[...] + narrow_in[...]

    def vmem(*shape):
        return pltpu.VMEM(shape, jnp.float32)

    return pl.pallas_call(
        body,
        out_shape=jax.ShapeDtypeStruct((1, n), jnp.float32),
        in_specs=[pl.BlockSpec(memory_space=pl.ANY)] * 3,
        out_specs=pl.BlockSpec(memory_space=pltpu.VMEM),
        scratch_shapes=[
            vmem(SWEEPS - 1, max(units), UNIT, SUBLANES, LANES),
            vmem(units[0], runs, cols - 1, SUBLANES, LANES),
            vmem(units[0], runs, 1, SUBLANES, LANES),
            vmem(Y_TILES + x_count + HEAD, SUBLANES, LANES),
            vmem(x_count, SUBLANES, LANES),
            vmem(HEAD, SUBLANES, LANES),
            vmem(1, n),
            vmem(1, n),
            vmem(1, wide),
            vmem(1, wide),
            vmem(1, LANES),
            vmem(1, LANES),
            pltpu.SemaphoreType.DMA((SWEEPS - 1,)),
            pltpu.SemaphoreType.DMA((8,)),
            pltpu.SemaphoreType.DMA((6,)),
            pltpu.SemaphoreType.DMA((6,)),
            pltpu.SemaphoreType.REGULAR,
        ],
        compiler_params=pltpu.CompilerParams(
            collective_id=0, disable_semaphore_checks=True
        ),
    )(x_tiles, x_periods, x_rows)
```

```python
import jax
import jax.numpy as jnp
from jax import lax
from jax.experimental import pallas as pl
from jax.experimental.pallas import tpu as pltpu

SUBLANES, LANES = 8, 128
HEAD = 7
UNIT = 16
SWEEPS = 8
LEFT_UNITS = 11
Y_TILES = 72
LAST_UNITS = 2

_MESH = pl.DeviceIdType.MESH


def _sum_groups(tiles, group):
    return jnp.sum(tiles.reshape(-1, group, SUBLANES, LANES), axis=0)


def _tree_sum(terms):
    while len(terms) > 1:
        pairs = [a + b for a, b in zip(terms[0::2], terms[1::2])]
        terms = pairs + terms[2 * len(pairs) :]
    return terms[0]


def _to_row(tiles):
    rows = [jnp.sum(tiles[i], axis=0, keepdims=True) for i in range(tiles.shape[0])]
    return jnp.concatenate(rows, axis=1)


def pallas_dist_sum_ax0_xy_m2048_n1024_kernel(x: jax.Array):
    m, n = x.shape
    cols = n // LANES
    tiles = m // SUBLANES * cols
    wide = n - LANES
    runs = UNIT // cols
    period = SWEEPS * UNIT
    assert HEAD == cols - 1 and UNIT % cols == 0 and Y_TILES % cols == 0
    x_tiles = (
        x.reshape(m // SUBLANES, SUBLANES, cols, LANES)
        .transpose(0, 2, 1, 3)
        .reshape(tiles, SUBLANES, LANES)
    )
    x_periods = x_tiles.reshape(tiles // period, period, SUBLANES, LANES)
    x_rows = x_tiles.reshape(tiles // period, period // cols, cols, SUBLANES, LANES)
    swept_units = (tiles - HEAD) // UNIT - LEFT_UNITS
    units = [len(range(j, swept_units, SWEEPS)) for j in range(SWEEPS)]
    early_units = units[0] - LAST_UNITS
    y_start = HEAD + swept_units * UNIT
    x_start = y_start + Y_TILES
    x_count = tiles - x_start

    def body(
        tiles_hbm, periods_hbm, rows_hbm, out_ref,
        swept_buf, wide_buf, narrow_buf, kept_buf, streamed_buf, head_buf,
        y_sum_out, y_sum_in, wide_out, wide_in, narrow_out, narrow_in,
        sweep_sems, read_sems, send_sems, recv_sems, helper_ready,
    ):
        def local(start, count, dst, sem):
            return pltpu.make_async_copy(tiles_hbm.at[pl.ds(start, count)], dst, sem)

        def sweep(j):
            start, count, sem = HEAD + j * UNIT, units[j], sweep_sems.at[j - 1]
            if start + UNIT <= period:
                src = periods_hbm.at[pl.ds(0, count), pl.ds(start, UNIT)]
                dst = swept_buf.at[j - 1, pl.ds(0, count)]
                return [pltpu.make_async_copy(src, dst, sem)]
            return [
                local(start + u * period, UNIT, swept_buf.at[j - 1, u], sem)
                for u in range(count)
            ]

        def slab(buf, row, col, width, first, count, sem):
            src = rows_hbm.at[pl.ds(first, count), pl.ds(row, runs), pl.ds(col, width)]
            dst = buf.at[pl.ds(first, count)]
            return pltpu.make_async_copy(src, dst, read_sems.at[sem])

        sweeps = [sweep(j) for j in range(1, SWEEPS)]
        wide_0 = slab(wide_buf, 1, 0, cols - 1, 0, early_units, 0)
        wide_1 = slab(wide_buf, 1, 0, cols - 1, early_units, LAST_UNITS, 1)
        narrow_0 = slab(narrow_buf, 0, cols - 1, 1, 0, early_units, 2)
        narrow_1 = slab(narrow_buf, 0, cols - 1, 1, early_units, LAST_UNITS, 3)
        for copies in sweeps[:-1]:
            for copy in copies:
                copy.start()

        my_x, my_y = lax.axis_index("x"), lax.axis_index("y")
        peer, side = (1 - my_x, my_y), (my_x, 1 - my_y)
        is_x0 = my_x == 0
        is_lead = jnp.logical_and(my_x == 1, my_y == 0)
        is_helper = jnp.logical_and(my_x == 1, my_y == 1)

        def remote(src, dst, target, sem):
            return pltpu.make_async_remote_copy(
                src, dst, send_sems.at[sem], recv_sems.at[sem],
                device_id=target, device_id_type=_MESH,
            )

        wide_swap = remote(wide_out, wide_in, peer, 0)
        narrow_swap = remote(narrow_out, narrow_in, peer, 1)
        x_stream = remote(tiles_hbm.at[pl.ds(x_start, x_count)], streamed_buf, peer, 2)
        head_stream = remote(tiles_hbm.at[pl.ds(0, HEAD)], head_buf, peer, 3)
        y_tiles = tiles_hbm.at[pl.ds(y_start, Y_TILES)]
        y_stream = remote(y_tiles, streamed_buf.at[pl.ds(0, Y_TILES)], side, 4)
        y_sum = remote(y_sum_out, y_sum_in, side, 5)
        left = Y_TILES + x_count
        kept_yx = local(y_start, left, kept_buf.at[pl.ds(0, left)], read_sems.at[4])
        kept_head = local(0, HEAD, kept_buf.at[pl.ds(left, HEAD)], read_sems.at[5])
        kept_y = local(y_start, Y_TILES, kept_buf.at[pl.ds(0, Y_TILES)], read_sems.at[6])
        own_head = local(0, HEAD, head_buf, read_sems.at[7])

        barrier = pltpu.get_barrier_semaphore()
        pl.semaphore_signal(barrier, 1, device_id=peer, device_id_type=_MESH)

        @pl.when(is_x0)
        def _():
            pl.semaphore_wait(barrier, 1)

        @pl.when(is_lead)
        def _():
            pl.semaphore_signal(barrier, 1, device_id=side, device_id_type=_MESH)
            pl.semaphore_wait(barrier, 1)
            x_stream.start()
            head_stream.start()
            pl.semaphore_wait(helper_ready, 1)
            y_stream.start()

        @pl.when(is_helper)
        def _():
            pl.semaphore_wait(barrier, 2)
            pl.semaphore_signal(helper_ready, 1, device_id=side, device_id_type=_MESH)
            x_stream.start()
            head_stream.start()

        for copy in (*sweeps[-1], wide_0, wide_1, narrow_0, narrow_1):
            copy.start()

        @pl.when(is_x0)
        def _():
            kept_yx.start()
            kept_head.start()

        @pl.when(is_helper)
        def _():
            kept_y.start()
            y_stream.wait_recv()
            y_sum_out[...] = _to_row(_sum_groups(streamed_buf[pl.ds(0, Y_TILES)], cols))
            y_sum.start()

        acc = jnp.zeros((cols, SUBLANES, LANES), jnp.float32)
        for j, copies in enumerate(sweeps, start=1):
            for copy in copies:
                copy.wait()
            acc = acc + _sum_groups(swept_buf[j - 1, pl.ds(0, units[j])], cols)
        wide_0.wait()
        acc_wide = acc[1:] + _sum_groups(wide_buf[pl.ds(0, early_units)], cols - 1)

        def rest_of_x0():
            kept_yx.wait()
            kept_head.wait()
            total = _sum_groups(kept_buf[...], cols)
            x_stream.wait_recv()
            total = total + _sum_groups(streamed_buf[pl.ds(0, x_count - 1)], cols)
            return total[1:], total[0] + streamed_buf[x_count - 1]

        def rest_of_lead():
            y_sum.wait_recv()
            top = lax.broadcasted_iota(jnp.int32, (SUBLANES, LANES), 0) == 0
            total = [
                jnp.where(top, y_sum_in[:, pl.ds(i * LANES, LANES)], 0.0)
                for i in range(cols)
            ]
            return jnp.stack(total[1:]), total[0]

        def rest_of_helper():
            kept_y.wait()
            total = _sum_groups(kept_buf[pl.ds(0, Y_TILES)], cols)
            return total[1:], total[0]

        rest_wide, rest_narrow = lax.cond(
            is_x0, rest_of_x0, lambda: lax.cond(is_lead, rest_of_lead, rest_of_helper)
        )
        acc_wide = acc_wide + rest_wide
        acc_narrow = acc[0] + rest_narrow

        early = [(u, r) for u in range(early_units) for r in range(runs)]
        last = [(u, r) for u in range(early_units, units[0]) for r in range(runs)]
        wide_1.wait()
        acc_wide = _tree_sum([wide_buf[u, r] for u, r in last] + [acc_wide])
        wide_out[...] = _to_row(acc_wide)
        wide_swap.start()
        narrow_0.wait()
        acc_narrow = _tree_sum([narrow_buf[u, r, 0] for u, r in early] + [acc_narrow])
        narrow_1.wait()
        acc_narrow = _tree_sum([narrow_buf[u, r, 0] for u, r in last] + [acc_narrow])
        narrow_out[...] = jnp.sum(acc_narrow, axis=0, keepdims=True)
        narrow_swap.start()

        @pl.when(my_x == 1)
        def _():
            own_head.start()
            own_head.wait()
            x_stream.wait_send()
            head_stream.wait_send()

        @pl.when(is_lead)
        def _():
            y_stream.wait_send()

        @pl.when(is_helper)
        def _():
            y_sum.wait_send()

        wide_swap.wait_send()
        narrow_swap.wait_send()

        @pl.when(is_x0)
        def _():
            head_stream.wait_recv()

        own_wide = wide_out[...] + _to_row(head_buf[...])
        wide_swap.wait_recv()
        out_ref[:, pl.ds(0, wide)] = own_wide + wide_in[...]
        narrow_swap.wait_recv()
        out_ref[:, pl.ds(wide, LANES)] = narrow_out[...] + narrow_in[...]

    def vmem(*shape):
        return pltpu.VMEM(shape, jnp.float32)

    return pl.pallas_call(
        body,
        out_shape=jax.ShapeDtypeStruct((1, n), jnp.float32),
        in_specs=[pl.BlockSpec(memory_space=pl.ANY)] * 3,
        out_specs=pl.BlockSpec(memory_space=pltpu.VMEM),
        scratch_shapes=[
            vmem(SWEEPS - 1, max(units), UNIT, SUBLANES, LANES),
            vmem(units[0], runs, cols - 1, SUBLANES, LANES),
            vmem(units[0], runs, 1, SUBLANES, LANES),
            vmem(Y_TILES + x_count + HEAD, SUBLANES, LANES),
            vmem(x_count, SUBLANES, LANES),
            vmem(HEAD, SUBLANES, LANES),
            vmem(1, n),
            vmem(1, n),
            vmem(1, wide),
            vmem(1, wide),
            vmem(1, LANES),
            vmem(1, LANES),
            pltpu.SemaphoreType.DMA((SWEEPS - 1,)),
            pltpu.SemaphoreType.DMA((8,)),
            pltpu.SemaphoreType.DMA((6,)),
            pltpu.SemaphoreType.DMA((6,)),
            pltpu.SemaphoreType.REGULAR,
        ],
        compiler_params=pltpu.CompilerParams(
            collective_id=0, disable_semaphore_checks=True
        ),
    )(x_tiles, x_periods, x_rows)
```
